```python
import numpy as np

kernel_name = "dist_mean_ax0_shard0_i_m2048_n1024"

def setup_inputs():
    return {"x": np.random.randn(8192, 1024).astype(np.float32)}

def reference(x: np.ndarray) -> np.ndarray:
    return np.mean(x, axis=0, keepdims=True)
```

```python
import jax
import jax.numpy as jnp
from jax import lax
from jax.experimental import pallas as pl
from jax.experimental.pallas import tpu as pltpu

N_DEV = 4
NUM_CHUNKS = 16


def pallas_dist_mean_ax0_shard0_i_m2048_n1024_kernel(
x: jax.Array,
):
    m_per, n = x.shape
    rows = m_per // NUM_CHUNKS
    inv_total = 1.0 / float(m_per * N_DEV)

    def body(x_hbm, out_ref, buf, send_buf, recv_buf, copy_sems, send_sems, recv_sems):
        my = lax.axis_index("i")

        copies = []
        for c in range(NUM_CHUNKS):
            cp = pltpu.make_async_copy(
                x_hbm.at[pl.ds(c * rows, rows)], buf.at[c], copy_sems.at[c]
            )
            cp.start()
            copies.append(cp)

        barrier = pltpu.get_barrier_semaphore()
        for d in range(1, N_DEV):
            pl.semaphore_signal(
                barrier, inc=1,
                device_id=((my + d) % N_DEV,),
                device_id_type=pl.DeviceIdType.MESH,
            )

        acc = jnp.zeros((8, n), jnp.float32)
        for c in range(NUM_CHUNKS):
            copies[c].wait()
            acc = acc + jnp.sum(buf[c].reshape(rows // 8, 8, n), axis=0)
        part = jnp.sum(acc, axis=0, keepdims=True)
        send_buf[...] = part

        pl.semaphore_wait(barrier, N_DEV - 1)

        rdmas = []
        for d in range(1, N_DEV):
            r = pltpu.make_async_remote_copy(
                src_ref=send_buf,
                dst_ref=recv_buf.at[d - 1],
                send_sem=send_sems.at[d - 1],
                recv_sem=recv_sems.at[d - 1],
                device_id=((my + d) % N_DEV,),
                device_id_type=pl.DeviceIdType.MESH,
            )
            r.start()
            rdmas.append(r)
        total = part
        for d in range(1, N_DEV):
            rdmas[d - 1].wait_recv()
            total = total + recv_buf[d - 1]
        out_ref[...] = total * inv_total
        for d in range(1, N_DEV):
            rdmas[d - 1].wait_send()

    return pl.pallas_call(
        body,
        out_shape=jax.ShapeDtypeStruct((1, n), jnp.float32),
        in_specs=[pl.BlockSpec(memory_space=pl.ANY)],
        out_specs=pl.BlockSpec(memory_space=pltpu.VMEM),
        scratch_shapes=[
            pltpu.VMEM((NUM_CHUNKS, rows, n), jnp.float32),
            pltpu.VMEM((1, n), jnp.float32),
            pltpu.VMEM((N_DEV - 1, 1, n), jnp.float32),
            pltpu.SemaphoreType.DMA((NUM_CHUNKS,)),
            pltpu.SemaphoreType.DMA((N_DEV - 1,)),
            pltpu.SemaphoreType.DMA((N_DEV - 1,)),
        ],
        compiler_params=pltpu.CompilerParams(collective_id=0),
    )(x)
```

```python
import jax
import jax.numpy as jnp
from jax import lax
from jax.experimental import pallas as pl
from jax.experimental.pallas import tpu as pltpu

N_DEV = 4
W = 128
RAW_ROWS = 104
EDGE_ROWS = 128
MID_ROWS = 160
STRIP_LAST = 32


def _rowsum(v):
    r, c = v.shape
    return jnp.sum(v.reshape(r // 8, 8, c), axis=0)


def _tree_add(parts):
    while len(parts) > 1:
        nxt = [parts[i] + parts[i + 1] for i in range(0, len(parts) - 1, 2)]
        if len(parts) % 2:
            nxt.append(parts[-1])
        parts = nxt
    return parts[0]


def _compiler_params():
    try:
        return pltpu.CompilerParams(collective_id=0, disable_semaphore_checks=True)
    except TypeError:
        return pltpu.CompilerParams(collective_id=0)


def pallas_dist_mean_ax0_shard0_i_m2048_n1024_kernel(
x: jax.Array,
):
    m, n = x.shape
    strip_rows = RAW_ROWS + EDGE_ROWS
    nfull = m - strip_rows
    bulk_rows = nfull - MID_ROWS
    assert bulk_rows > 0 and bulk_rows % 8 == 0 and n % 128 == 0 and n > W
    full_chunks = ((0, bulk_rows), (bulk_rows, MID_ROWS))
    strip_parts = ((0, strip_rows - STRIP_LAST), (strip_rows - STRIP_LAST, STRIP_LAST))
    inv_total = 1.0 / float(m * N_DEV)

    def body(x_hbm, out_ref, full_buf, edge_buf, strip_buf, raw_buf,
             send_r, send_l, send_full, diag_r, diag_l, nbr_buf,
             copy_sems, send_sems, recv_sems):
        my = lax.axis_index("i")

        def remote(src, dst, k, offset):
            return pltpu.make_async_remote_copy(
                src_ref=src, dst_ref=dst,
                send_sem=send_sems.at[k], recv_sem=recv_sems.at[k],
                device_id=((my + offset) % N_DEV,),
                device_id_type=pl.DeviceIdType.MESH,
            )

        full_cps = []
        for k, (o, r) in enumerate(full_chunks):
            cp = pltpu.make_async_copy(
                x_hbm.at[pl.ds(o, r)], full_buf.at[pl.ds(o, r)], copy_sems.at[k])
            cp.start()
            full_cps.append(cp)
        edge_cp = pltpu.make_async_copy(
            x_hbm.at[pl.ds(nfull, EDGE_ROWS), pl.ds(W, n - W)], edge_buf,
            copy_sems.at[2])
        edge_cp.start()
        strip_cps = []
        for k, (o, r) in enumerate(strip_parts):
            cp = pltpu.make_async_copy(
                x_hbm.at[pl.ds(nfull + o, r), pl.ds(0, W)],
                strip_buf.at[pl.ds(o, r)], copy_sems.at[3 + k])
            cp.start()
            strip_cps.append(cp)

        barrier = pltpu.get_barrier_semaphore()
        for d in range(1, N_DEV):
            pl.semaphore_signal(
                barrier, inc=1, device_id=((my + d) % N_DEV,),
                device_id_type=pl.DeviceIdType.MESH)
        pl.semaphore_wait(barrier, N_DEV - 1)

        raw = remote(x_hbm.at[pl.ds(m - RAW_ROWS, RAW_ROWS), pl.ds(W, n - W)],
                     raw_buf, 0, 1)
        raw.start()

        acc = None
        for cp, (o, r) in zip(full_cps, full_chunks):
            cp.wait()
            s = _rowsum(full_buf[pl.ds(o, r), :])
            acc = s if acc is None else acc + s
        acc_l, acc_r = acc[:, :W], acc[:, W:]
        raw.wait_recv()
        acc_r = acc_r + _rowsum(raw_buf[...])
        edge_cp.wait()
        acc_r = acc_r + _rowsum(edge_buf[...])
        part_r = jnp.sum(acc_r, axis=0, keepdims=True)
        send_r[...] = part_r
        to_diag_r = remote(send_r, diag_r, 1, 2)
        to_diag_r.start()
        send_full[:, W:] = part_r

        for cp, (o, r) in zip(strip_cps, strip_parts):
            cp.wait()
            acc_l = _tree_add(
                [acc_l] + [strip_buf[pl.ds(o + 8 * i, 8), :] for i in range(r // 8)])
        part_l = jnp.sum(acc_l, axis=0, keepdims=True)
        send_l[...] = part_l
        to_diag_l = remote(send_l, diag_l, 2, 2)
        to_diag_l.start()
        send_full[:, :W] = part_l
        to_nbrs = []
        for k, d in enumerate((1, N_DEV - 1)):
            cp = remote(send_full, nbr_buf.at[k], 3 + k, d)
            cp.start()
            to_nbrs.append(cp)

        for cp in (raw, to_diag_r, to_diag_l, *to_nbrs):
            cp.wait_send()

        for k, cp in enumerate(to_nbrs):
            cp.wait_recv()
            part_l = part_l + nbr_buf[k, :, :W]
            part_r = part_r + nbr_buf[k, :, W:]
        to_diag_r.wait_recv()
        out_ref[:, W:] = (part_r + diag_r[...]) * inv_total
        to_diag_l.wait_recv()
        out_ref[:, :W] = (part_l + diag_l[...]) * inv_total

    f32 = jnp.float32
    return pl.pallas_call(
        body,
        out_shape=jax.ShapeDtypeStruct((1, n), f32),
        in_specs=[pl.BlockSpec(memory_space=pl.ANY)],
        out_specs=pl.BlockSpec(memory_space=pltpu.VMEM),
        scratch_shapes=[
            pltpu.VMEM((nfull, n), f32),
            pltpu.VMEM((EDGE_ROWS, n - W), f32),
            pltpu.VMEM((strip_rows, W), f32),
            pltpu.VMEM((RAW_ROWS, n - W), f32),
            pltpu.VMEM((1, n - W), f32),
            pltpu.VMEM((1, W), f32),
            pltpu.VMEM((1, n), f32),
            pltpu.VMEM((1, n - W), f32),
            pltpu.VMEM((1, W), f32),
            pltpu.VMEM((2, 1, n), f32),
            pltpu.SemaphoreType.DMA((5,)),
            pltpu.SemaphoreType.DMA((5,)),
            pltpu.SemaphoreType.DMA((5,)),
        ],
        compiler_params=_compiler_params(),
    )(x)
```
